```python
import numpy as np

kernel_name = "dist_ring_attn_i_s256_d64"

def setup_inputs():
    S, D = 1024, 64
    q = np.random.randn(S, D).astype(np.float32)
    k = np.random.randn(S, D).astype(np.float32)
    v = np.random.randn(S, D).astype(np.float32)
    return {"q": q, "k": k, "v": v}

def reference(q: np.ndarray, k: np.ndarray, v: np.ndarray) -> np.ndarray:
    D = q.shape[1]
    scores = q @ k.T / np.sqrt(D)
    scores_max = np.max(scores, axis=1, keepdims=True)
    weights = np.exp(scores - scores_max)
    weights = weights / np.sum(weights, axis=1, keepdims=True)
    return weights @ v
```

```python
import math

import jax
import jax.numpy as jnp
from jax import lax
from jax.experimental import pallas as pl
from jax.experimental.pallas import tpu as pltpu

N_DEV = 4
S_LOC = 256
D = 64
H = 128
SCALE = math.log2(math.e) / math.sqrt(D)
BF = jnp.bfloat16
F32 = jnp.float32
MESH = pl.DeviceIdType.MESH

NCH = 8
CH = D // NCH

OWN_K, OWN_V, FST_K, FST_V, SND_K, SND_V, THD_K, THD_V = range(8)


def _body(qT_hbm, kT_hbm, vT_hbm, oT_ref, q_v, k_v, v_v, kv,
          in_sems, rdy_sem, send_sem, fst_sems, grp_sems):
    my = lax.axis_index("i")
    left = (my + N_DEV - 1) % N_DEV
    right = (my + 1) % N_DEV
    nbr = (right, left)
    is_odd = (my % 2) == 1

    bar = pltpu.get_barrier_semaphore()

    @pl.when(my != 2)
    def _():
        for nb in nbr:
            pl.semaphore_signal(bar, inc=1, device_id=(nb,), device_id_type=MESH)

    k_loads = [
        pltpu.make_async_copy(kT_hbm.at[pl.ds(c * CH, CH)], k_v.at[pl.ds(c * CH, CH)], in_sems.at[2 + c])
        for c in range(NCH)
    ]
    for c in k_loads:
        c.start()
    v_load = pltpu.make_async_copy(vT_hbm, v_v, in_sems.at[0])
    v_load.start()
    q_load = pltpu.make_async_copy(qT_hbm, q_v, in_sems.at[1])
    q_load.start()

    def rcopy(src, dst, recv_sem, d):
        return pltpu.make_async_remote_copy(
            src, dst, send_sem, recv_sem, device_id=(nbr[d],), device_id_type=MESH)

    def first(d, part, c):
        rows = pl.ds(c * CH, CH)
        return rcopy(kv.at[OWN_K + part, d, rows], kv.at[FST_K + part, d, rows],
                     fst_sems.at[(d * 2 + part) * NCH + c], d)

    def second(d, part):
        return rcopy(kv.at[OWN_K + part, 1 - d], kv.at[SND_K + part, d], grp_sems.at[part], d)

    def relay(d, part, c):
        rows = pl.ds(c * CH, CH)
        return rcopy(kv.at[FST_K + part, d, rows], kv.at[THD_K + part, d, rows],
                     grp_sems.at[2 + part], d)

    def wait_group(g, sem):
        pltpu.make_async_copy(kv.at[g], kv.at[g], sem).wait()

    def towards_ready(fn):
        pl.when(my != 1)(lambda: fn(0))
        pl.when(my != 3)(lambda: fn(1))

    @pl.when(my == 2)
    def _():
        pl.semaphore_wait(bar, 2)
        for nb in nbr:
            pl.semaphore_signal(rdy_sem, inc=1, device_id=(nb,), device_id_type=MESH)

    for c in range(NCH):
        k_loads[c].wait()
        kc = k_v[pl.ds(c * CH, CH), :].astype(BF)
        kv[OWN_K, 0, pl.ds(c * CH, CH)] = kc[:, :H]
        kv[OWN_K, 1, pl.ds(c * CH, CH)] = kc[:, H:]
        if c == 0:
            pl.when(my == 0)(lambda: pl.semaphore_wait(bar, 2))
            pl.when(is_odd)(lambda: pl.semaphore_wait(bar, 1))
        towards_ready(lambda d, c=c: first(d, 0, c).start())

    v_load.wait()
    vb = v_v[...].astype(BF)
    kv[OWN_V, 0] = vb[:, :H]
    kv[OWN_V, 1] = vb[:, H:]

    def send_rest(d):
        for c in range(NCH):
            first(d, 1, c).start()
        second(d, 0).start()
        second(d, 1).start()

    def send_all(d):
        pl.semaphore_wait(rdy_sem, 1)
        for c in range(NCH):
            first(d, 0, c).start()
        send_rest(d)

    towards_ready(send_rest)

    q_load.wait()
    qs = (q_v[...] * SCALE).astype(BF)

    def k_phase(g, carry):
        sts = [jnp.dot(kv[g, j].T, qs, preferred_element_type=F32) for j in (0, 1)]
        m_blk = jnp.maximum(jnp.max(sts[0], axis=0, keepdims=True),
                            jnp.max(sts[1], axis=0, keepdims=True))
        if carry is None:
            m_new = m_blk
        else:
            m, l, acc = carry
            m_new = jnp.maximum(m, m_blk)
            alpha = jnp.exp2(m - m_new)
        ps = [jnp.exp2(st - m_new) for st in sts]
        l_blk = jnp.sum(ps[0], axis=0, keepdims=True) + jnp.sum(ps[1], axis=0, keepdims=True)
        pb = [p.astype(BF) for p in ps]
        if carry is None:
            return m_new, l_blk, None, pb
        return m_new, alpha * l + l_blk, alpha * acc, pb

    def v_phase(g, acc, pb):
        for j in (0, 1):
            pv = jnp.dot(kv[g, j], pb[j], preferred_element_type=F32)
            acc = pv if acc is None else acc + pv
        return acc

    m, l, acc, pb = k_phase(OWN_K, None)
    acc = v_phase(OWN_V, None, pb)

    pl.when(my == 1)(lambda: send_all(0))
    pl.when(my == 3)(lambda: send_all(1))

    for part in (0, 1):
        for c in range(NCH):
            for d in (0, 1):
                first(d, part, c).wait_recv()
                relay(d, part, c).start()

    m, l, acc, pb = k_phase(FST_K, (m, l, acc))
    acc = v_phase(FST_V, acc, pb)

    wait_group(SND_K, grp_sems.at[0])
    m, l, acc, pb = k_phase(SND_K, (m, l, acc))
    wait_group(SND_V, grp_sems.at[1])
    acc = v_phase(SND_V, acc, pb)

    wait_group(THD_K, grp_sems.at[2])
    m, l, acc, pb = k_phase(THD_K, (m, l, acc))
    wait_group(THD_V, grp_sems.at[3])
    acc = v_phase(THD_V, acc, pb)

    oT_ref[...] = acc * (1.0 / l)

    pltpu.make_async_copy(kv.at[0:6], kv.at[0:6], send_sem).wait()


def pallas_dist_ring_attn_i_s256_d64_kernel(
    q: jax.Array,
    k: jax.Array,
    v: jax.Array,
):
    out = pl.pallas_call(
        _body,
        out_shape=jax.ShapeDtypeStruct((D, S_LOC), F32),
        in_specs=[pl.BlockSpec(memory_space=pl.ANY)] * 3,
        out_specs=pl.BlockSpec(memory_space=pltpu.VMEM),
        scratch_shapes=[
            pltpu.VMEM((D, S_LOC), F32),
            pltpu.VMEM((D, S_LOC), F32),
            pltpu.VMEM((D, S_LOC), F32),
            pltpu.VMEM((8, 2, D, H), BF),
            pltpu.SemaphoreType.DMA((2 + NCH,)),
            pltpu.SemaphoreType.REGULAR,
            pltpu.SemaphoreType.DMA,
            pltpu.SemaphoreType.DMA((4 * NCH,)),
            pltpu.SemaphoreType.DMA((4,)),
        ],
        compiler_params=pltpu.CompilerParams(collective_id=0, disable_semaphore_checks=True),
    )(q.T, k.T, v.T)
    return out.T
```
